```python
import numpy as np

kernel_name = "dist_pipemlp_pp2tp2_xy_b4096_d256_h512"

def setup_inputs():
    x_padded = np.zeros((2, 4096, 256), dtype=np.float32)
    x_padded[0] = np.random.randn(4096, 256).astype(np.float32)
    Win = np.random.randn(4, 256, 1024).astype(np.float32)
    Wout = np.random.randn(4, 1024, 256).astype(np.float32)
    return {"x_padded": x_padded, "Win": Win, "Wout": Wout}

def reference(x_padded, Win, Wout):
    a = x_padded[0]
    for k in range(4):
        h = a @ Win[k]
        h = np.maximum(h, 0.0)
        a = h @ Wout[k]
    out = np.zeros_like(x_padded)
    out[1] = a
    return out
```

```python
import functools

import jax
import jax.numpy as jnp
from jax import lax
from jax.experimental import pallas as pl
from jax.experimental.pallas import tpu as pltpu

_BF16 = jnp.bfloat16
_F32 = jnp.float32

_Q = 256
_L0_ROWS = 512
_ACT_ROWS = 64
_OUT_ROWS = 128
_OWN_FIRST = 512
_FIRST_CUTS = ((32, 96, 128), (128, 128))
_VIA = (64, 64, 48, 48)
_STEPS = (
    (0, 1, 5, True, 0, 2),
    (0, 5, 1, False, 2, 3),
    (5, 1, 3, True, 0, 3),
    (0, 2, 1, False, 3, 4),
    (2, 6, 1, False, 3, 4),
    (8, 2, 2, True, 0, 4),
    (12, 1, 4, True, 0, 4),
)
_EARLY_ROWS = 64
_DETOUR = {4: 48, 5: 128, 6: 128, 7: 128, 8: 128, 10: 112}
_HOPS = [(c * _OUT_ROWS + r, min(_ACT_ROWS, n - r))
         for c, n in _DETOUR.items() for r in range(0, n, _ACT_ROWS)]
_HOPS_IN_LOOP = 4


def _loop(n, body):
    if n == 1:
        body(0)
    else:
        lax.fori_loop(0, n, lambda i, c: body(i), None)


def _when(cond, body):
    if not isinstance(cond, bool):
        pl.when(cond)(body)
    elif cond:
        body()


def _rows(start, n, align):
    return pl.ds(start if isinstance(start, int) else pl.multiple_of(start, align), n)


def _kernel(
    x_hbm, win_hbm, wout_hbm, out_ref,
    wf, wi, wo, wvia, xbuf, pown, psnd, prcv, act, a3, p3, early, osnd, orcv, hop1, hop2,
    wld_sem, xld_sem, wsnd_sem, wrcv_sem, vsnd_sem, vrcv_sem, psnd_sem, prcv_sem,
    asnd_sem, arcv_sem, early_sem, osnd_sem, orcv_sem,
    h1rcv_sem, h2snd_sem, h2rcv_sem, h3snd_sem, h3rcv_sem, entered_sem,
):
    half, d = x_hbm.shape[1] // 2, x_hbm.shape[2]
    mx, my = lax.axis_index("x"), lax.axis_index("y")
    x_nbr, y_nbr = (1 - mx, my), (mx, 1 - my)
    own0, oth0 = my * half, (1 - my) * half

    def remote(src, dst, send_sem, recv_sem, to):
        return pltpu.make_async_remote_copy(
            src, dst, send_sem, recv_sem,
            device_id=to, device_id_type=pl.DeviceIdType.MESH)

    def ffn(v, l, q0, q1):
        h = jnp.dot(v, wi[l, :, q0 * _Q:q1 * _Q], preferred_element_type=_F32)
        h = jnp.maximum(h, 0.0).astype(_BF16)
        return jnp.dot(h, wo[l, q0 * _Q:q1 * _Q, :], preferred_element_type=_F32)

    def w_parts(l, shared_first):
        parts = []
        for q in range(2):
            for io in range(2):
                cuts = _FIRST_CUTS[io] if shared_first and q == 0 else (_Q,)
                parts += [(l, q, io, sum(cuts[:k]), n) for k, n in enumerate(cuts)]
        return parts

    def w_load(part, k):
        l, q, io, r0, n = part
        if io == 0:
            src = win_hbm.at[l, pl.ds(r0, n), pl.ds(q * _Q, _Q)]
        else:
            src = wout_hbm.at[l, pl.ds(q * _Q + r0, n), :]
        return pltpu.make_async_copy(src, wf.at[l, q, io, pl.ds(r0, n)], wld_sem.at[k])

    def w_cast(part):
        l, q, io, r0, n = part
        v = wf[l, q, io, pl.ds(r0, n)].astype(_BF16)
        if io == 0:
            wi[l, pl.ds(r0, n), pl.ds(q * _Q, _Q)] = v
        else:
            wo[l, pl.ds(q * _Q + r0, n), :] = v

    def w_view(part, theirs):
        l, q, io, r0, n = part
        h0 = (2 * theirs + q) * _Q
        if io == 0:
            return wi.at[l, pl.ds(r0, n), pl.ds(h0, _Q)]
        return wo.at[l, pl.ds(h0 + r0, n), :]

    def w_send(part, k):
        return remote(w_view(part, 0), w_view(part, 1),
                      wsnd_sem.at[k], wrcv_sem.at[k], y_nbr)

    def share(part, k):
        w_load(part, k).wait()
        w_cast(part)
        w_send(part, k).start()

    vias = [(1, 1, 1, _Q - sum(_VIA[:m + 1]), n) for m, n in enumerate(_VIA)]

    def via_copy(m, hop):
        stop = [wvia.at[k, pl.ds(*vias[m][3:])] for k in range(2)]
        src = (w_view(vias[m], 0), stop[0], stop[1])[hop]
        dst = (stop[0], stop[1], w_view(vias[m], 1))[hop]
        return remote(src, dst, vsnd_sem.at[3 * m + hop], vrcv_sem.at[3 * m + hop],
                      (x_nbr, y_nbr, x_nbr)[hop])

    def each_via(from_y, body):
        for m in range(len(vias) - 1):
            body(m)
        pl.when(from_y == 1)(lambda: body(len(vias) - 1))

    def act_copy(i):
        r = _rows(i * _ACT_ROWS, _ACT_ROWS, _ACT_ROWS)
        return remote(act.at[r], act.at[r], asnd_sem, arcv_sem.at[i], x_nbr)

    def out_copy(i, skip=0):
        r = _rows(i * _OUT_ROWS + skip, _OUT_ROWS - skip, _OUT_ROWS)
        return remote(osnd.at[r], orcv.at[r], osnd_sem, orcv_sem.at[i], y_nbr)

    def hop1_copy(j):
        r = pl.ds(*_HOPS[j])
        return remote(osnd.at[r], hop1.at[r], osnd_sem, h1rcv_sem.at[j], x_nbr)

    def hop2_copy(j):
        r = pl.ds(*_HOPS[j])
        return remote(hop1.at[r], hop2.at[r], h2snd_sem.at[j], h2rcv_sem.at[j], y_nbr)

    def hop3_copy(j):
        r = pl.ds(*_HOPS[j])
        return remote(hop2.at[r], orcv.at[r], h3snd_sem.at[j], h3rcv_sem.at[j], x_nbr)

    n_win, n_wout = (len(cuts) for cuts in _FIRST_CUTS)
    n_piece0 = n_win + n_wout
    urgent = w_parts(1 - mx, True)
    for k in range(n_win):
        w_load(urgent[k], k).start()

    barrier = pltpu.get_barrier_semaphore()
    pl.semaphore_signal(
        barrier, inc=1, device_id=y_nbr, device_id_type=pl.DeviceIdType.MESH)

    @pl.when(mx == 0)
    def _():
        pl.semaphore_signal(
            barrier, inc=1, device_id=x_nbr, device_id_type=pl.DeviceIdType.MESH)

    for k in range(n_win):
        w_load(urgent[k], k).wait()
        w_cast(urgent[k])
        if k == 0:
            for j in range(n_win, n_piece0):
                w_load(urgent[j], j).start()
            for j, part in enumerate(w_parts(mx, False)):
                w_load(part, len(urgent) + j).start()
            pl.when(mx == 0)(lambda: pl.semaphore_wait(barrier, 1))
            pl.when(mx == 1)(lambda: pl.semaphore_wait(barrier, 2))
        w_send(urgent[k], k).start()

    @pl.when(mx == 0)
    def _stage0():
        shared, local = w_parts(1, True), w_parts(0, False)
        shared[-1] = shared[-1][:4] + (_Q - sum(_VIA),)
        tail, k_tail = (1, 1, 1, _Q - sum(_VIA), sum(_VIA)), len(shared + local)
        n_blocks, n_steps = half // _L0_ROWS, half // _ACT_ROWS

        def x_load(b):
            start = lax.rem(oth0 + b * _L0_ROWS, 2 * half)
            return pltpu.make_async_copy(
                x_hbm.at[0, _rows(start, _L0_ROWS, _L0_ROWS)],
                xbuf.at[_rows(b * _L0_ROWS, _L0_ROWS, _L0_ROWS)], xld_sem.at[b])

        def part_copy(i):
            r = _rows(i * _ACT_ROWS, _ACT_ROWS, _ACT_ROWS)
            return remote(psnd.at[r], prcv.at[r], psnd_sem, prcv_sem.at[i], y_nbr)

        def their_block(b, loads):
            x_load(b).wait()
            for copy in loads:
                copy.start()
            r = _rows(b * _L0_ROWS, _L0_ROWS, _L0_ROWS)
            psnd[r] = ffn(xbuf[r].astype(_BF16), 0, 0, 2).astype(_BF16)

        def send_block(b):
            per = _L0_ROWS // _ACT_ROWS
            for k in range(per):
                part_copy(b * per + k).start()

        def own_rows(r0, n):
            v = xbuf[_rows(half + r0, n, 16)].astype(_BF16)
            pown[_rows(r0, n, 16)] = ffn(v, 0, 0, 2)

        w_load(tail, k_tail).start()
        x_load(0).start()
        w_load(tail, k_tail).wait()
        w_cast(tail)
        pl.semaphore_wait(entered_sem, 1)
        each_via(my, lambda m: via_copy(m, 0).start())
        pl.when(my == 0)(lambda: w_send(vias[-1], k_tail).start())
        for k in range(n_win, n_piece0):
            share(shared[k], k)
        for k, part in enumerate(local):
            w_load(part, len(shared) + k).wait()
            w_cast(part)

        rest = range(n_piece0, len(shared))
        their_block(0, [x_load(1)] + [w_load(shared[k], k) for k in rest])
        for k in rest:
            share(shared[k], k)
        send_block(0)

        def next_block(b):
            their_block(b, [x_load(2 * b), x_load(2 * b + 1)])
            send_block(b)

        _loop(n_blocks - 1, lambda b: next_block(b + 1))

        n_late = (half - _OWN_FIRST) // (n_steps // 2)
        assert n_late % 16 == 0 and _OWN_FIRST + n_late * (n_steps // 2) == half
        assert all(_OWN_FIRST + t * n_late >= 2 * t * _ACT_ROWS
                   for t in range(1, n_steps // 2 + 1))
        x_load(n_blocks).wait()
        own_rows(0, _OWN_FIRST)
        for b in range(n_blocks + 1, 2 * n_blocks):
            x_load(b).wait()
        own_rows(_OWN_FIRST, n_late)

        each_via(1 - my, lambda m: via_copy(m, 2).wait_recv())
        pl.when(my == 1)(lambda: w_send(vias[-1], k_tail).wait_recv())
        for k, part in enumerate(shared):
            w_send(part, k).wait_recv()

        def forward(j):
            hop1_copy(j).wait_recv()
            hop2_copy(j).start()

        def step(i, parity):
            for j in range(_HOPS_IN_LOOP):
                at = n_steps - _HOPS_IN_LOOP + j
                if at % 2 == parity:
                    pl.when(i == at)(functools.partial(forward, j))
            r = _rows(i * _ACT_ROWS, _ACT_ROWS, _ACT_ROWS)
            part_copy(i).wait_recv()
            a1 = (pown[r] + prcv[r].astype(_F32)).astype(_BF16)
            act[r] = ffn(a1, 1, 0, 4).astype(_BF16)
            act_copy(i).start()

        def two_steps(t):
            step(2 * t, 0)
            step(2 * t + 1, 1)
            pl.when(t + 1 < n_steps // 2)(
                lambda: own_rows(_OWN_FIRST + (t + 1) * n_late, n_late))

        _loop(n_steps // 2, two_steps)

        for k, part in enumerate(shared):
            w_send(part, k).wait_send()
        remote(psnd, prcv, psnd_sem, prcv_sem.at[0], y_nbr).wait_send()
        each_via(my, lambda m: via_copy(m, 0).wait_send())
        pl.when(my == 0)(lambda: w_send(vias[-1], k_tail).wait_send())

        n_zero = 8
        assert len(_HOPS) >= n_zero
        for j in range(len(_HOPS)):
            hop2_copy(j).wait_recv()
            hop3_copy(j).start()
            if _HOPS_IN_LOOP + j < len(_HOPS):
                forward(_HOPS_IN_LOOP + j)
            if j < n_zero:
                n = 2 * half // n_zero
                out_ref[0, pl.ds(j * n, n)] = jnp.zeros((n, d), _F32)
        remote(act, act, asnd_sem, arcv_sem.at[0], x_nbr).wait_send()
        for j in range(len(_HOPS)):
            hop2_copy(j).wait_send()
        for j in range(len(_HOPS)):
            hop3_copy(j).wait_send()

    @pl.when(mx == 1)
    def _stage1():
        shared = w_parts(0, True) + w_parts(1, False)
        pl.semaphore_signal(
            entered_sem, inc=1, device_id=x_nbr, device_id_type=pl.DeviceIdType.MESH)

        def pass_on(m, hop):
            via_copy(m, hop - 1).wait_recv()
            via_copy(m, hop).start()

        for k in range(n_piece0, len(urgent)):
            w_load(shared[k], k).start()
        for k in range(n_win, len(shared)):
            if k == n_win + 1:
                each_via(my, lambda m: pass_on(m, 1))
            share(shared[k], k)
        each_via(1 - my, lambda m: pass_on(m, 2))

        here = []

        def need_weights(l, q1):
            for k, part in enumerate(shared):
                if part[0] == l and 2 + part[1] < q1 and k not in here:
                    here.append(k)
                    w_send(part, k).wait_recv()

        def send(i, may_be):
            def among(chunks):
                hits = [c for c in may_be if c in chunks]
                if len(hits) in (0, len(may_be)):
                    return bool(hits)
                return functools.reduce(jnp.logical_or, [i == c for c in hits])

            def split(c):
                if _DETOUR[c] < _OUT_ROWS:
                    out_copy(c, _DETOUR[c]).start()
                for j, (r0, _) in enumerate(_HOPS):
                    if r0 // _OUT_ROWS == c:
                        hop1_copy(j).start()

            _when(among([c for c in may_be if c and c not in _DETOUR]),
                  lambda: out_copy(i).start())
            _when(among([0]), lambda: out_copy(0, _EARLY_ROWS).start())
            for c in _DETOUR:
                _when(among([c]), functools.partial(split, c))

        def step(c0, m, n, layer2, q0, q1, t):
            i = c0 + t * m
            r = _rows(i * _OUT_ROWS, m * _OUT_ROWS, _OUT_ROWS)
            if layer2:
                per = _OUT_ROWS // _ACT_ROWS
                for k in range(m * per):
                    act_copy(i * per + k).wait_recv()
                v = ffn(act[r], 0, 0, 4).astype(_BF16)
                if q1 < 4:
                    a3[r] = v
            else:
                v = a3[r]
            o = ffn(v, 1, q0, q1)
            if q0:
                o += p3[r]
            if q1 < 4:
                p3[r] = o
                return
            osnd[r] = o.astype(_BF16)
            for k in range(m):
                send(i + k, range(c0 + k, c0 + n * m, m))

        inputs, sums = pl.ds(0, _EARLY_ROWS), pl.ds(_EARLY_ROWS, _EARLY_ROWS)
        early_copy = remote(early.at[0], early.at[1], early_sem.at[0], early_sem.at[1], y_nbr)

        for c0, m, n, layer2, q0, q1 in _STEPS:
            need_weights(0, 4)
            need_weights(1, q1)
            _loop(n, functools.partial(step, c0, m, n, layer2, q0, q1))
            if c0 == 0 and q1 == 3:
                partial = p3[inputs].astype(_BF16)
                p3[inputs] = partial.astype(_F32)
                early[0, inputs] = a3[inputs]
                early[0, sums] = partial
                early_copy.start()

        early_copy.wait()
        o = early[1, sums].astype(_F32) + ffn(early[1, inputs], 1, 1, 2)
        out_ref[0, _rows(oth0, _EARLY_ROWS, 16)] = o.astype(_BF16).astype(_F32)
        out_ref[0, _rows(own0, half, 16)] = osnd[...].astype(_F32)
        for k, part in enumerate(shared):
            w_send(part, k).wait_send()
        each_via(my, lambda m: via_copy(m, 1).wait_send())
        each_via(1 - my, lambda m: via_copy(m, 2).wait_send())

        skip = {0: _EARLY_ROWS, **_DETOUR}
        direct = [(out_copy(i, skip.get(i, 0)), i * _OUT_ROWS + skip.get(i, 0),
                   _OUT_ROWS - skip.get(i, 0))
                  for i in range(half // _OUT_ROWS) if skip.get(i, 0) < _OUT_ROWS]
        around = [(hop3_copy(j), r0, n) for j, (r0, n) in enumerate(_HOPS)]
        while direct or around:
            left = [sum(msg[2] for msg in queue) for queue in (direct, around)]
            copy, r0, n = (direct if left[0] >= left[1] else around).pop(0)
            copy.wait_recv()
            out_ref[0, _rows(oth0 + r0, n, 16)] = orcv[pl.ds(r0, n)].astype(_F32)
        r = pl.ds(_EARLY_ROWS, half - _EARLY_ROWS)
        remote(osnd.at[r], orcv.at[r], osnd_sem, orcv_sem.at[0], y_nbr).wait_send()


def pallas_dist_pipemlp_pp2tp2_xy_b4096_d256_h512_kernel(
    x_padded: jax.Array,
    Win: jax.Array,
    Wout: jax.Array,
):
    _, rows, d = x_padded.shape
    assert (rows, d) == (4096, _Q)
    assert Win.shape == (2, d, 2 * _Q) and Wout.shape == (2, 2 * _Q, d)
    half = rows // 2
    n_weights = sum(len(cuts) for cuts in _FIRST_CUTS) + 7
    dma = pltpu.SemaphoreType.DMA
    hbm = pl.BlockSpec(memory_space=pltpu.HBM)
    return pl.pallas_call(
        _kernel,
        out_shape=pltpu.VMEM(x_padded.shape, _F32),
        in_specs=[hbm, hbm, hbm],
        out_specs=pl.BlockSpec(memory_space=pltpu.VMEM),
        scratch_shapes=[
            pltpu.VMEM((2, 2, 2, _Q, _Q), _F32),
            pltpu.VMEM((2, d, 4 * _Q), _BF16),
            pltpu.VMEM((2, 4 * _Q, d), _BF16),
            pltpu.VMEM((2, _Q, d), _BF16),
            pltpu.VMEM((rows, d), _F32),
            pltpu.VMEM((half, d), _F32),
            pltpu.VMEM((half, d), _BF16),
            pltpu.VMEM((half, d), _BF16),
            pltpu.VMEM((half, d), _BF16),
            pltpu.VMEM((half, d), _BF16),
            pltpu.VMEM((half, d), _F32),
            pltpu.VMEM((2, 2 * _EARLY_ROWS, d), _BF16),
            pltpu.VMEM((half, d), _BF16),
            pltpu.VMEM((half, d), _BF16),
            pltpu.VMEM((half, d), _BF16),
            pltpu.VMEM((half, d), _BF16),
            dma((n_weights,)),
            dma((rows // _L0_ROWS,)),
            dma((n_weights,)),
            dma((n_weights,)),
            dma((3 * len(_VIA),)),
            dma((3 * len(_VIA),)),
            dma,
            dma((half // _ACT_ROWS,)),
            dma,
            dma((half // _ACT_ROWS,)),
            dma((2,)),
            dma,
            dma((half // _OUT_ROWS,)),
            dma((len(_HOPS),)),
            dma((len(_HOPS),)),
            dma((len(_HOPS),)),
            dma((len(_HOPS),)),
            dma((len(_HOPS),)),
            pltpu.SemaphoreType.REGULAR,
        ],
        compiler_params=pltpu.CompilerParams(
            collective_id=0,
            vmem_limit_bytes=48 * 1024 * 1024,
            disable_semaphore_checks=True,
        ),
    )(x_padded, Win, Wout)
```
